```python
import numpy as np

kernel_name = "dist_sum_ax0_xy_m2048_n1024"

def setup_inputs():
    return {"x": np.random.randn(4096, 2048).astype(np.float32)}

def reference(x: np.ndarray) -> np.ndarray:
    return np.sum(x, axis=0, keepdims=True)
```

```python
import jax
import jax.numpy as jnp
from jax import lax
from jax.experimental import pallas as pl
from jax.experimental.pallas import tpu as pltpu

_MESH = pl.DeviceIdType.MESH

_KX = 96
_KS = 48
_BIG = (512, 512, 512)
_TAIL = (96, 32)
_B_SPLIT = (144, 16)
_G = 128


def _tree_sum(vs):
    vs = list(vs)
    while len(vs) > 1:
        nxt = [vs[i] + vs[i + 1] for i in range(0, len(vs) - 1, 2)]
        if len(vs) % 2:
            nxt.append(vs[-1])
        vs = nxt
    return vs[0]


def pallas_dist_sum_ax0_xy_m2048_n1024_kernel(
    x: jax.Array,
):
    m, n = x.shape
    r_last = sum(_B_SPLIT)
    rem = m - _KX - _KS - r_last - sum(_BIG) - sum(_TAIL)
    assert rem > 0 and rem % 8 == 0 and n % 128 == 0 and n > _G
    main = _BIG + (rem,) + _TAIL
    na = n - _G
    nm = sum(main)
    moff = [sum(main[:i]) for i in range(len(main))]
    boff = [sum(_B_SPLIT[:i]) for i in range(len(_B_SPLIT))]
    s_row = nm + r_last
    x_row = s_row + _KS

    def kernel_body(x_hbm, out_ref, buf, abuf, bbuf, smem, sbuf, raw,
                    send_a, send_b, recv_a, recv_b,
                    sems, hop_sems, send_sems, recv_sems):
        cm = [
            pltpu.make_async_copy(
                x_hbm.at[pl.ds(moff[i], r)], buf.at[pl.ds(moff[i], r)], sems.at[i])
            for i, r in enumerate(main)
        ]
        ca = pltpu.make_async_copy(
            x_hbm.at[pl.ds(nm, r_last), pl.ds(0, na)], abuf, sems.at[len(main)])
        cb = [
            pltpu.make_async_copy(
                x_hbm.at[pl.ds(nm + boff[i], r), pl.ds(na, _G)],
                bbuf.at[pl.ds(boff[i], r)],
                sems.at[len(main) + 1 + i])
            for i, r in enumerate(_B_SPLIT)
        ]
        hop1 = pltpu.make_async_copy(x_hbm.at[pl.ds(s_row, _KS)], smem, hop_sems.at[0])
        hop2 = pltpu.make_async_copy(smem, sbuf, hop_sems.at[1])

        cm[0].start()
        hop1.start()

        nbr = (1 - lax.axis_index("x"), lax.axis_index("y"))
        barrier = pltpu.get_barrier_semaphore()
        pl.semaphore_signal(barrier, inc=1, device_id=nbr, device_id_type=_MESH)

        ca.start()
        for c in cm[1:] + cb:
            c.start()

        pl.semaphore_wait(barrier, 1)

        def remote(src, dst, k):
            return pltpu.make_async_remote_copy(
                src, dst, send_sems.at[k], recv_sems.at[k],
                device_id=nbr, device_id_type=_MESH)

        r_raw = remote(x_hbm.at[pl.ds(x_row, _KX)], raw, 0)
        r_raw.start()

        def psum(ref, a, r):
            v = ref[pl.ds(a, r), :]
            return jnp.sum(v.reshape(r // 8, 8, v.shape[1]), axis=0)

        cm[0].wait()
        acc = psum(buf, moff[0], main[0])
        hop1.wait()
        hop2.start()
        ca.wait()
        acc_a = acc[:, :na] + psum(abuf, 0, r_last)
        acc_b = acc[:, na:]
        for i in range(1, len(main)):
            cm[i].wait()
            v = psum(buf, moff[i], main[i])
            if i == 2:
                hop2.wait()
                v = v + psum(sbuf, 0, _KS)
            if i == 3:
                r_raw.wait()
                v = v + psum(raw, 0, _KX)
            acc_a = acc_a + v[:, :na]
            acc_b = acc_b + v[:, na:]

        send_a[...] = jnp.sum(acc_a, axis=0, keepdims=True)
        r_a = remote(send_a, recv_a, 1)
        r_a.start()

        for i, r in enumerate(_B_SPLIT):
            cb[i].wait()
            acc_b = _tree_sum(
                [bbuf[pl.ds(boff[i] + 8 * j, 8), :] for j in range(r // 8)] + [acc_b])
        part_b = jnp.sum(acc_b, axis=0, keepdims=True)
        send_b[...] = part_b
        r_b = remote(send_b, recv_b, 2)
        r_b.start()

        r_a.wait_send()
        r_b.wait_send()
        r_a.wait_recv()
        out_ref[:, pl.ds(0, na)] = send_a[...] + recv_a[...]
        r_b.wait_recv()
        out_ref[:, pl.ds(na, _G)] = part_b + recv_b[...]

    f32 = jnp.float32
    return pl.pallas_call(
        kernel_body,
        out_shape=jax.ShapeDtypeStruct((1, n), f32),
        in_specs=[pl.BlockSpec(memory_space=pl.ANY)],
        out_specs=pl.BlockSpec(memory_space=pltpu.VMEM),
        scratch_shapes=[
            pltpu.VMEM((nm, n), f32),
            pltpu.VMEM((r_last, na), f32),
            pltpu.VMEM((r_last, _G), f32),
            pltpu.SMEM((_KS, n), f32),
            pltpu.VMEM((_KS, n), f32),
            pltpu.VMEM((_KX, n), f32),
            pltpu.VMEM((1, na), f32),
            pltpu.VMEM((1, _G), f32),
            pltpu.VMEM((1, na), f32),
            pltpu.VMEM((1, _G), f32),
            pltpu.SemaphoreType.DMA((len(main) + 1 + len(_B_SPLIT),)),
            pltpu.SemaphoreType.DMA((2,)),
            pltpu.SemaphoreType.DMA((3,)),
            pltpu.SemaphoreType.DMA((3,)),
        ],
        compiler_params=pltpu.CompilerParams(
            collective_id=0,
            vmem_limit_bytes=32 * 1024 * 1024,
            disable_semaphore_checks=True,
        ),
    )(x)
```

```python
import jax
import jax.numpy as jnp
from jax import lax
from jax.experimental import pallas as pl
from jax.experimental.pallas import tpu as pltpu

_MESH = pl.DeviceIdType.MESH

_KX = 96
_KS = 48
_BIG = (512, 512, 448)
_TAIL = (96, 32)
_B_SPLIT = (224, 32)
_G = 128


def _tree_sum(vs):
    vs = list(vs)
    while len(vs) > 1:
        nxt = [vs[i] + vs[i + 1] for i in range(0, len(vs) - 1, 2)]
        if len(vs) % 2:
            nxt.append(vs[-1])
        vs = nxt
    return vs[0]


def _compiler_params():
    kw = dict(collective_id=0, vmem_limit_bytes=32 * 1024 * 1024)
    try:
        return pltpu.CompilerParams(disable_semaphore_checks=True, **kw)
    except TypeError:
        return pltpu.CompilerParams(**kw)


def pallas_dist_sum_ax0_xy_m2048_n1024_kernel(
    x: jax.Array,
):
    m, n = x.shape
    r_last = sum(_B_SPLIT)
    rem = m - _KX - _KS - r_last - sum(_BIG) - sum(_TAIL)
    assert rem > 0 and rem % 8 == 0 and n % 128 == 0 and n > _G
    main = _BIG + (rem,) + _TAIL
    na = n - _G
    nm = sum(main)
    moff = [sum(main[:i]) for i in range(len(main))]
    boff = [sum(_B_SPLIT[:i]) for i in range(len(_B_SPLIT))]
    s_row = nm + r_last
    x_row = s_row + _KS

    def kernel_body(x_hbm, out_ref, buf, abuf, bbuf, smem, sbuf, raw,
                    send_a, send_b, recv_a, recv_b,
                    sems, hop_sems, send_sems, recv_sems):
        cm = [
            pltpu.make_async_copy(
                x_hbm.at[pl.ds(moff[i], r)], buf.at[pl.ds(moff[i], r)], sems.at[i])
            for i, r in enumerate(main)
        ]
        ca = pltpu.make_async_copy(
            x_hbm.at[pl.ds(nm, r_last), pl.ds(0, na)], abuf, sems.at[len(main)])
        cb = [
            pltpu.make_async_copy(
                x_hbm.at[pl.ds(nm + boff[i], r), pl.ds(na, _G)],
                bbuf.at[pl.ds(boff[i], r)],
                sems.at[len(main) + 1 + i])
            for i, r in enumerate(_B_SPLIT)
        ]
        hop1 = pltpu.make_async_copy(x_hbm.at[pl.ds(s_row, _KS)], smem, hop_sems.at[0])
        hop2 = pltpu.make_async_copy(smem, sbuf, hop_sems.at[1])

        cm[0].start()
        hop1.start()

        nbr = (1 - lax.axis_index("x"), lax.axis_index("y"))
        barrier = pltpu.get_barrier_semaphore()
        pl.semaphore_signal(barrier, inc=1, device_id=nbr, device_id_type=_MESH)

        ca.start()
        for c in cm[1:] + cb:
            c.start()

        pl.semaphore_wait(barrier, 1)

        def remote(src, dst, k):
            return pltpu.make_async_remote_copy(
                src, dst, send_sems.at[k], recv_sems.at[k],
                device_id=nbr, device_id_type=_MESH)

        r_raw = remote(x_hbm.at[pl.ds(x_row, _KX)], raw, 0)
        r_raw.start()

        def psum(ref, a, r):
            v = ref[pl.ds(a, r), :]
            return jnp.sum(v.reshape(r // 8, 8, v.shape[1]), axis=0)

        cm[0].wait()
        acc = psum(buf, moff[0], main[0])
        hop1.wait()
        hop2.start()
        ca.wait()
        acc_a = acc[:, :na] + psum(abuf, 0, r_last)
        acc_b = acc[:, na:]
        for i in range(1, len(main)):
            cm[i].wait()
            v = psum(buf, moff[i], main[i])
            if i == 2:
                hop2.wait()
                v = v + psum(sbuf, 0, _KS)
            if i == 3:
                r_raw.wait()
                v = v + psum(raw, 0, _KX)
            acc_a = acc_a + v[:, :na]
            acc_b = acc_b + v[:, na:]

        send_a[...] = jnp.sum(acc_a, axis=0, keepdims=True)
        r_a = remote(send_a, recv_a, 1)
        r_a.start()

        for i, r in enumerate(_B_SPLIT):
            cb[i].wait()
            acc_b = _tree_sum(
                [bbuf[pl.ds(boff[i] + 8 * j, 8), :] for j in range(r // 8)] + [acc_b])
        part_b = jnp.sum(acc_b, axis=0, keepdims=True)
        send_b[...] = part_b
        r_b = remote(send_b, recv_b, 2)
        r_b.start()

        r_a.wait_send()
        r_b.wait_send()
        r_a.wait_recv()
        out_ref[:, pl.ds(0, na)] = send_a[...] + recv_a[...]
        r_b.wait_recv()
        out_ref[:, pl.ds(na, _G)] = part_b + recv_b[...]

    f32 = jnp.float32
    return pl.pallas_call(
        kernel_body,
        out_shape=jax.ShapeDtypeStruct((1, n), f32),
        in_specs=[pl.BlockSpec(memory_space=pl.ANY)],
        out_specs=pl.BlockSpec(memory_space=pltpu.VMEM),
        scratch_shapes=[
            pltpu.VMEM((nm, n), f32),
            pltpu.VMEM((r_last, na), f32),
            pltpu.VMEM((r_last, _G), f32),
            pltpu.SMEM((_KS, n), f32),
            pltpu.VMEM((_KS, n), f32),
            pltpu.VMEM((_KX, n), f32),
            pltpu.VMEM((1, na), f32),
            pltpu.VMEM((1, _G), f32),
            pltpu.VMEM((1, na), f32),
            pltpu.VMEM((1, _G), f32),
            pltpu.SemaphoreType.DMA((len(main) + 1 + len(_B_SPLIT),)),
            pltpu.SemaphoreType.DMA((2,)),
            pltpu.SemaphoreType.DMA((3,)),
            pltpu.SemaphoreType.DMA((3,)),
        ],
        compiler_params=_compiler_params(),
    )(x)
```
